```python
import numpy as np

kernel_name = "dist_mlp2_tp_i_m512_h1024_out512"

def setup_inputs():
    x = np.random.randn(512, 512).astype(np.float32)
    W1 = np.random.randn(512, 4096).astype(np.float32)
    W2 = np.random.randn(4096, 512).astype(np.float32)
    return {"x": x, "W1": W1, "W2": W2}

def reference(x: np.ndarray, W1: np.ndarray, W2: np.ndarray) -> np.ndarray:
    h = x @ W1
    h = np.maximum(h, 0.0)
    return h @ W2
```

```python
import contextlib
import jax
import jax.numpy as jnp
from jax import lax
from jax.experimental import pallas as pl
from jax.experimental.pallas import tpu as pltpu

MESH = pl.DeviceIdType.MESH
F32, BF16 = jnp.float32, jnp.bfloat16


def make(prof=False, w1mode="k", cast=True):
    scope = (lambda n: jax.named_scope(n)) if prof else (lambda n: contextlib.nullcontext())

    def body(x_hbm, w1_hbm, w2_hbm, out, xv, w1v, w2v, xb, w1b, w2b, hacc, hb, sb, r1, kb, r2, lsem, ssem, rsem):
        me = lax.axis_index("i")
        p1 = me ^ 1
        p2 = 3 - me
        k1 = jnp.where((me == 0) | (me == 3), 0, 1)
        k2 = jnp.where(me < 2, 2, 3)
        s1 = 1 - k1
        s2 = 5 - k2
        blk = lambda b: pl.ds(pl.multiple_of(b * 128, 128), 128)

        loads = []

        def load(src, dst):
            cp = pltpu.make_async_copy(src, dst, lsem.at[len(loads)])
            cp.start()
            loads.append(cp)
            return cp

        lx = [load(x_hbm.at[blk(s1)], xv.at[pl.ds(0, 128)]), load(x_hbm.at[blk(s2)], xv.at[pl.ds(128, 128)])]
        if w1mode == "k":
            lw1 = [load(w1_hbm.at[pl.ds(k * 128, 128)], w1v.at[pl.ds(k * 128, 128)]) for k in range(4)]
        else:
            lw1 = [load(w1_hbm.at[:, pl.ds(c * 256, 256)], w1v.at[:, pl.ds(c * 256, 256)]) for c in range(4)]
        lw2 = [[load(w2_hbm.at[pl.ds(k * 512, 512), pl.ds(0, 128)], w2v.at[pl.ds(k * 512, 512), pl.ds(0, 128)]) for k in range(2)]]
        for c in range(1, 4):
            lw2.append([load(w2_hbm.at[:, pl.ds(c * 128, 128)], w2v.at[:, pl.ds(c * 128, 128)])])
            if c == 2:
                lx.append(load(x_hbm.at[blk(k1)], xv.at[pl.ds(256, 128)]))
        lx.append(load(x_hbm.at[blk(k2)], xv.at[pl.ds(384, 128)]))

        bar = pltpu.get_barrier_semaphore()
        for n in (p1, p2):
            pl.semaphore_signal(bar, inc=1, device_id=(n,), device_id_type=MESH)

        sends = []

        def send(src, dst, slot, dev):
            cp = pltpu.make_async_remote_copy(src, dst, ssem, rsem.at[slot], device_id=(dev,), device_id_type=MESH)
            cp.start()
            sends.append(cp)

        def recv(dst, slot):
            pltpu.make_async_remote_copy(dst, dst, ssem, rsem.at[slot], device_id=(me,), device_id_type=MESH).wait_recv()

        with scope("wx"):
            lx[0].wait()
            lx[1].wait()
        xb[0:256] = xv[0:256].astype(BF16)
        for k in range(4):
            with scope(f"ww1_{k}"):
                lw1[k].wait()
            with scope(f"h_{k}"):
                if w1mode == "k":
                    ks = pl.ds(k * 128, 128)
                    w = w1v[ks, :].astype(BF16)
                    w1b[ks, :] = w
                    d = jnp.dot(xb[0:256, ks], w, preferred_element_type=F32)
                    if k == 0:
                        hacc[...] = d
                    elif k < 3:
                        hacc[...] += d
                    else:
                        hb[0:256] = jnp.maximum(hacc[...] + d, 0.0).astype(BF16)
                else:
                    cs = pl.ds(k * 256, 256)
                    w = w1v[:, cs].astype(BF16)
                    w1b[:, cs] = w
                    d = jnp.dot(xb[0:256], w, preferred_element_type=F32)
                    hb[0:256, cs] = jnp.maximum(d, 0.0).astype(BF16)
        with scope("bar"):
            pl.semaphore_wait(bar, 2)
        for c in range(4):
            cs = pl.ds(c * 128, 128)
            acc = None
            n = len(lw2[c])
            for k in range(n):
                with scope(f"ww2_{c}_{k}"):
                    lw2[c][k].wait()
                with scope(f"o_{c}_{k}"):
                    ks = pl.ds(k * (1024 // n), 1024 // n)
                    w = w2v[ks, cs].astype(BF16)
                    w2b[ks, cs] = w
                    d = jnp.dot(hb[0:256, ks], w, preferred_element_type=F32)
                    acc = d if acc is None else acc + d
                    if k == n - 1:
                        sb[c] = acc.astype(BF16)
            send(sb.at[c, pl.ds(0, 128)], r1.at[c, pl.ds(0, 128)], c, p1)
            send(sb.at[c, pl.ds(128, 128)], r1.at[c, pl.ds(128, 128)], 4 + c, p2)
            if c == 2:
                with scope("wx2"):
                    lx[2].wait()
                with scope("h2"):
                    d = jnp.dot(xv[256:384].astype(BF16), w1b[...], preferred_element_type=F32)
                    hb[256:384] = jnp.maximum(d, 0.0).astype(BF16)
        with scope("wx3"):
            lx[3].wait()
        with scope("h3"):
            d = jnp.dot(xv[384:512].astype(BF16), w1b[...], preferred_element_type=F32)
            hb[384:512] = jnp.maximum(d, 0.0).astype(BF16)
        for c in range(4):
            cs = pl.ds(c * 128, 128)
            with scope(f"r1_{c}"):
                recv(r1.at[c, pl.ds(0, 128)], c)
                recv(r1.at[c, pl.ds(128, 128)], 4 + c)
            with scope(f"ok_{c}"):
                d = jnp.dot(hb[256:512], w2b[:, cs], preferred_element_type=F32)
                kb[c] = (d + r1[c].astype(F32)).astype(BF16)
            send(kb.at[c, pl.ds(0, 128)], r2.at[c, pl.ds(0, 128)], 8 + c, p2)
            send(kb.at[c, pl.ds(128, 128)], r2.at[c, pl.ds(128, 128)], 12 + c, p1)
        for c in range(4):
            cs = pl.ds(c * 128, 128)
            with scope(f"r2_{c}"):
                recv(r2.at[c, pl.ds(0, 128)], 8 + c)
                recv(r2.at[c, pl.ds(128, 128)], 12 + c)
            t = (kb[c].astype(F32) + r2[c].astype(F32)).astype(BF16)
            out[blk(k1), cs] = t[0:128]
            out[blk(k2), cs] = t[128:256]
            send(out.at[blk(k1), cs], out.at[blk(k1), cs], 16, p1)
            send(out.at[blk(k2), cs], out.at[blk(k2), cs], 17, p2)
        with scope("wsend"):
            for cp in sends:
                cp.wait_send()
        with scope("r3"):
            recv(out.at[blk(s1)], 16)
            recv(out.at[blk(s2)], 17)

    def f(x, W1, W2):
        hbm = pl.BlockSpec(memory_space=pltpu.HBM)
        return pl.pallas_call(
            body,
            out_shape=jax.ShapeDtypeStruct((512, 512), BF16),
            in_specs=[hbm] * 3,
            out_specs=pl.BlockSpec(memory_space=pltpu.VMEM),
            scratch_shapes=[
                pltpu.VMEM((512, 512), F32), pltpu.VMEM((512, 1024), F32), pltpu.VMEM((1024, 512), F32),
                pltpu.VMEM((512, 512), BF16), pltpu.VMEM((512, 1024), BF16), pltpu.VMEM((1024, 512), BF16),
                pltpu.VMEM((256, 1024), F32), pltpu.VMEM((512, 1024), BF16),
                pltpu.VMEM((4, 256, 128), BF16), pltpu.VMEM((4, 256, 128), BF16),
                pltpu.VMEM((4, 256, 128), BF16), pltpu.VMEM((4, 256, 128), BF16),
                pltpu.SemaphoreType.DMA((16,)), pltpu.SemaphoreType.DMA, pltpu.SemaphoreType.DMA((18,)),
            ],
            compiler_params=pltpu.CompilerParams(collective_id=0, disable_semaphore_checks=True, disable_bounds_checks=True,
                                                 vmem_limit_bytes=48 << 20),
        )(x, W1, W2)

    return f


def pallas_dist_mlp2_tp_i_m512_h1024_out512_kernel(x, W1, W2):
    return make()(x, W1, W2)
```

```python
import jax
import jax.numpy as jnp
from jax import lax
from jax.experimental import pallas as pl
from jax.experimental.pallas import tpu as pltpu

FIRST, SIDE, LAST = 0, 1, 2
ROWS, HALF, LANES, HIDDEN = 32, 256, 128, 1024
OPENING = 8
F32, BF16 = jnp.float32, jnp.bfloat16

VIA_FIRST = "l0123.0 l0123.1 l123.2"

PLANS = {
    FIRST: """
        | X4567.0123 X01.0123 W.12 ! | s1.2 W.0 s0.2 vs1.1 s4.0 s01.3 s567.0 s45.3 s67.3
        vs01.3 vs1.0 h014567.1 W.3 vs01.2 | Y.0 h014567.2 Y.1 h014567.0 | Y.2 h04567.3 Y.3
        m6.0 ~ m7.0 p6.0 ~ m45.0 p7.0 ~ h1.3 p45.0 | m5.1 ~ m6.1 p5.1 m7.1 | p67.1 |
        X23.0123 | ~ m14.1 p4.1 m7.2 ~ m0.2 p7.2 ~ m6.2 p0.2 m45.2 ~ m0.1 p456.2 ~ m01.0 |
        p01.0 m01.3 ~ m46.3 p1.3 p0.3 m57.3 p0.1 p4567.3 p1.1 h23.0123 m23.3 ~ m3.0 p23.3 |
        m2.0 f23.0 p23.0 | ~ m1.2 m23.12 p23.1 p123.2 | f123.2 f0123.1 | f45.1 | f01.3 f0.2
        | f2.3 f6.2 | f6.1 f6.3
    """,
    SIDE: """
        | X234567.12 X01.1 W.12 ! | s234.1 W.0 | s1.1 s0.1 | W.3 h012345.1 ~ h67.1 s23.2 Y.0
        | Y.1 s4.2 s01.2 h01234567.2 vh1.1 | s01.3 s4.0 Y.2 h014.0 vh0.0 Y.3 h23567.0 s4.3
        vX7.0123 | h145.3 vh23.0 | h02367.3 | m34.0 ~ m067.0 l4.0 l3.0 ~ m125.0 l67.0 l0.0 ~
        vh0123.3 vX4.0123 l5.0 l1.0 l2.0 | m16.1 ~ m045.1 l1.1 l6.1 vX5.0123 ~ m237.1 l0.1
        l4.1 ~ vh1.02 vh2.1 l23.1 l7.1 l5.1 vh3.12 | m34.2 ~ m125.2 l4.2 l3.2 m0.2 ~ m6.2
        vh2.2 l12.2 l0.2 l5.2 vh0.12 ~ vm123.0 l6.2 | a1.0 m0.3 ~ m134.3 l0.3 vX6.0123 a2.0
        ~ vm0.0 l34.3 l1.3 | a3.0 ~ vm0123.1 a0.0 ~ m2.3 | a1.1 | a0.1 l2.3 m567.3 ~ vh4.0
        l56.3 | a2.1 ~ vm12.2 a3.1 l7.3 vh4.123 a2.2 ~ vm3.2 a1.2 c01.0 vh5.0 vm4.0 ~ vm4.1
        | a4.0 c4.1 c4.0 | ~ m7.2 vm4.2 a3.2 vh5.123 a4.1 | l7.2 | c4.2 a4.2 vm05.2 ~ vm5.01
        c5.0 | a0.2 c5.2 ~ vm05.3 a5.1 vm134.3 a5.0 | c1.1 a5.2 c0.2 c5.3 vh7.0123 | a0.3 |
        ~ vm2.3 vm7.23 a4.3 c0.3 vh6.1 a3.3 ~ vm7.1 c7.2 a1.3 c34.3 vh6.023 a2.3 c7.1 | a5.3
        vm6.2 ~ vm6.3 | c7.3 c2.3 a6.2 | a6.3 vm6.1 ~ vm67.0 | c67.0 a6.1 | c3.1 a6.0 | c6.2
        c5.1 c2.1 c0.1 c23.0 c2.2 a7.0 | a7.2 | a7.3 c6.3 c1.3 c1.2 | c3.2 c6.1 a7.1 |
    """,
    LAST: """
        | X0123.0 W.0 ! vs0.0 X23.3 W.1 | s01.0 s23.0 vs23.0 | W.23 | s23.3 h0123.0 | vs23.3
        vs23.1 ~ h23.1 | Y.0 | h4.1 ~ h01.1 Y.1 | Y.2 vs23.2 h234.2 vs0.1 X5.0123 | h01.2 |
        Y.3 | X67.0123 h0123.3 | m1.0 ~ m2.0 p1.0 ~ m03.0 p2.0 ~ h4.0 p3.0 h4.3 p0.0 m1.1 ~
        m0.1 p1.1 ~ m2.1 p0.1 ~ m3.1 m4.01 p2.1 | p3.1 | m2.2 ~ m1.2 p2.2 ~ m3.2 p1.2 ~ m4.2
        p4.0 p3.2 | ~ m0.2 p4.1 h5.0123 | p4.2 ~ m5.1 p0.2 ~ m03.3 p5.1 m5.0 ~ m5.2 p5.0 |
        p5.2 p0.3 h6.2 m14.3 p4.3 p3.3 ~ m25.3 p1.3 h6.013 p2.3 | ~ m6.2 p5.3 ~ m6.3 h7.0
        p6.2 ~ m6.01 p6.3 ~ h7.12 p6.1 p6.0 h7.3 m7.0 ~ m7.2 p7.0 | p7.2 m7.3 ~ m7.1 p7.3 |
        p7.1 f01.0 | f5.0 f45.2 | f5.3 f4.0 | f34.3 f7.2 f7.1 | f7.0 f7.3 f6.0
    """,
}


def _tokens(plan):
    for word in plan.split():
        hub = word[0] == "v"
        groups, _, blocks = word[hub + 1:].partition(".")
        yield word[hub], hub, [int(g) for g in groups], [int(b) for b in blocks]


def _spans(starts, step):
    spans = []
    for start in sorted(starts):
        if spans and sum(spans[-1]) == start and start != HALF:
            spans[-1] = (spans[-1][0], spans[-1][1] + step)
        else:
            spans.append((start, step))
    return spans


def _route(plans, via_first):
    first = {(g, j) for _, _, groups, blocks in _tokens(via_first) for g in groups for j in blocks}
    runs, inbox = {role: [] for role in plans}, {role: [] for role in plans}
    for role, plan in plans.items():
        kind, totals = None, set()
        for op, hub, groups, blocks in _tokens(plan):
            if role == SIDE:
                rows = [g * ROWS + HALF * (hub or op in "ac") for g in groups]
            else:
                rows = [g * ROWS + half for half in (0, HALF) for g in groups]
            previous, kind = kind, "mxu" if op in "hm~" else "send" if op in "slpacf" else op
            if kind != previous:
                runs[role].append((kind, []))
            if kind != "send":
                runs[role][-1][1].append((op, rows, blocks))
                continue
            for j in blocks:
                routes = {}
                for r in rows:
                    leaf = 1 if r < HALF else 3
                    via = FIRST if (r % HALF // ROWS, j) in first else LAST
                    if op == "s":
                        route = "x", LAST if role == SIDE else leaf ^ (2 * hub), "x"
                    elif op == "l":
                        route = "part", via, "other"
                    elif op == "p":
                        route = "part", leaf ^ 2, "rest" if via == role else "other"
                    elif op == "f":
                        route = "out", leaf, "out"
                    else:
                        to = FIRST if op == "a" else LAST
                        if to != via:
                            totals.add((r, j))
                        route = ("out", to, "out") if (r, j) in totals else ("part", to, "rest")
                    routes.setdefault(route, []).append(r)
                for (src, to, dst), starts in routes.items():
                    for r, n in _spans(starts, ROWS):
                        runs[role][-1][1].append((src, (role, to, dst, r, n, j)))
                        if role == SIDE:
                            inbox[to] += [(1, to, dst, r, n, j), (3, to, dst, r ^ HALF, n, j)]
                        elif to == 1:
                            inbox[SIDE].append((role, 1, dst, r, n, j))
    return runs, inbox


def _program(role, runs, inbox):
    def slot(message):
        sender, to, dst, r, n, j = message
        if to == 3:
            return inbox[SIDE].index((sender, 1, dst, r ^ HALF, n, j))
        return inbox[to].index(message)

    source, ready = {}, set()
    for index, (_, _, dst, r, n, j) in enumerate(inbox[role]):
        source.update({(dst, q, j): ("recv", index, dst, r, n, j) for q in range(r, r + n, ROWS)})

    def need(name, r, j, waits, work):
        if (name, r, j) in ready:
            return
        ready.add((name, r, j))
        wait = source.get((name, r, j))
        if wait is not None:
            if wait not in ready:
                ready.add(wait)
                waits.append(wait)
            if name == "x" and wait[0] == "loaded":
                work.append(("cast", r, j))
        elif name == "part":
            need("other", r, j, waits, work)
            work.append(("add", r, j))
        else:
            assert name == "out", (role, name, r, j)
            need("part", r, j, waits, work)
            need("rest", r, j, waits, work)
            work.append(("total", r, j))

    steps, loads, depth, held = [], 0, {}, set()
    for kind, items in runs:
        waits, work, tail = [], [], []
        if not held:
            wait_at = len(steps)
        if kind == "!":
            waits.append(("barrier",))
        elif kind == "|":
            work.append(("store",))
            held = set()
        elif kind == "send":
            for src, message in items:
                _, to, dst, r, n, j = message
                for q in range(r, r + n, ROWS):
                    if src != "x" and (q, j) in held:
                        work.insert(0, ("store",))
                        held = set()
                    need(src, q, j, waits, work)
                tail.append(("send", slot(message), to, src, dst, r, n, j))
        elif kind == "mxu":
            work.append(("store",))
            dots, hold, held = {}, False, set()
            for op, rows, blocks in items:
                hold = hold or op == "~"
                for key in [tuple(blocks)] if op == "h" else blocks:
                    for r in rows:
                        dots.setdefault((op, key, r in depth or op == "m", hold), []).append(r)
            for (op, key, started, hold), rows in dots.items():
                if op == "h":
                    for k in key:
                        need("w1", 0, k, waits, work)
                        for r in rows:
                            need("x", r, k, waits, work)
                            depth[r] = depth.get(r, 0) + 1
                    done = [r for r in rows if depth[r] == 4]
                    held.update(rows if hold else [])
                    tail.append(("hidden", hold, sorted(rows), key, started, done))
                else:
                    assert all(depth[r] == 4 and r not in held for r in rows), (role, rows)
                    need("w2", 0, key, waits, work)
                    alone = [r for r in rows if ("other", r, key) not in source]
                    fused = [r for r in rows if source.get(("other", r, key)) in ready]
                    ready.update(("part", r, key) for r in alone + fused)
                    held.update((r, key) for r in rows if hold)
                    tail.append(("partial", hold, sorted(rows), key, alone, fused))
        else:
            name = {"X": "x", "W": "w1", "Y": "w2"}[kind]
            for _, rows, blocks in items:
                for rs, bs in [(rows, blocks)] if name == "x" else [([0], [b]) for b in blocks]:
                    tail.append(("load", loads, name, rs, bs))
                    source.update({(name, r, b): ("loaded", loads) for r in rs for b in bs})
                    loads += 1
        steps[wait_at:wait_at] = waits
        wait_at += len(waits)
        steps += work + tail

    last = []
    for _, _, dst, r, n, j in inbox[role]:
        waits, work = [], []
        for q in range(r, r + n, ROWS):
            if dst in ("rest", "out"):
                need("out", q, j, waits, work)
        last += waits + work
    every = [(r, b) for r in range(0, 2 * HALF, ROWS) for b in range(4)]
    assert sorted((r, k) for s in steps if s[0] == "hidden" for r in s[2] for k in s[3]) == every
    assert sorted((r, s[3]) for s in steps if s[0] == "partial" for r in s[2]) == every
    assert ready.issuperset(("out", r, j) for r, j in every)
    assert ready.issuperset(source.values()) and not held
    return steps + [("drain", 8)] + last[:-2] + [("drain", 0)] + last[-2:]


def _schedule(plans, via_first):
    runs, inbox = _route(plans, via_first)
    return {role: _program(role, runs[role], inbox) for role in plans}


def _build(programs):
    count = lambda kind: max(sum(step[0] == kind for step in p) for p in programs.values())

    def body(x_hbm, w1_hbm, w2_hbm, out, x_f32, w1, w2, x, h_acc, h, acc, part, other, rest,
             load_sems, send_sems, recv_sems):
        opening = pltpu.make_async_copy(
            w1_hbm.at[:OPENING], w1.at[:OPENING, :HIDDEN], load_sems.at[count("load")])
        opening.start()

        me = lax.axis_index("i")
        mirrored = (me == 3).astype(jnp.int32)
        mesh = pl.DeviceIdType.MESH
        barrier = pltpu.get_barrier_semaphore()
        for neighbour in ((me + 1) & 3, (me + 3) & 3):
            pl.semaphore_signal(barrier, 1, device_id=(neighbour,), device_id_type=mesh)

        def global_row(role, r):
            if role != SIDE:
                return r
            return pl.multiple_of(r + mirrored * ((r ^ HALF) - r), ROWS)

        def tile(name, r, n, j):
            if name == "out":
                return out.at[pl.ds(r, n), pl.ds(j * LANES, LANES)]
            return {"x": x, "part": part, "other": other, "rest": rest}[name].at[j, pl.ds(r, n)]

        def load(role, index, name, rows, blocks):
            copy = lambda src, dst: pltpu.make_async_copy(src, dst, load_sems.at[index])
            block = pl.ds(blocks[0] * LANES, LANES)
            if name == "w1":
                if blocks[0] == 0:
                    block = pl.ds(OPENING, LANES - OPENING)
                return [copy(w1_hbm.at[block], w1.at[block, :HIDDEN])]
            if name == "w2":
                return [copy(w2_hbm.at[:, pl.ds(q, 16), block], w2.at[blocks[0], :, pl.ds(q, 16)])
                        for q in range(0, 64, 16)]
            return [
                copy(x_hbm.at[pl.ds(global_row(role, r), n), pl.ds(c * LANES, m * LANES)],
                     x_f32.at[pl.ds(r, n), pl.ds(c * LANES, m * LANES)])
                for c, m in _spans(blocks, 1) for r, n in _spans(rows, ROWS)
            ]

        def gather(ref, rows, blocks):
            return jnp.concatenate(
                [jnp.concatenate([ref[b, pl.ds(r, n)] for b in blocks], axis=1)
                 for r, n in _spans(rows, ROWS)], axis=0)

        def hidden(rows, ks, started, done):
            weights = [w1[pl.ds(k * LANES, LANES), :HIDDEN].astype(BF16) for k in ks]
            product = jnp.dot(gather(x, rows, ks), jnp.concatenate(weights, axis=0),
                              preferred_element_type=F32)

            def store():
                for i, r in enumerate(rows):
                    value = product[i * ROWS:(i + 1) * ROWS]
                    if started:
                        value = value + h_acc[pl.ds(r, ROWS), :HIDDEN]
                    if r in done:
                        value = jnp.maximum(value, 0.0).astype(BF16)
                        for n in range(HIDDEN // LANES):
                            h[n, pl.ds(r, ROWS)] = value[:, n * LANES:(n + 1) * LANES]
                    else:
                        h_acc[pl.ds(r, ROWS), :HIDDEN] = value

            return store

        def partial(rows, j, alone, fused):
            weights = w2[j].reshape(HIDDEN, LANES).astype(BF16)
            product = jnp.dot(gather(h, rows, range(HIDDEN // LANES)), weights,
                              preferred_element_type=F32)

            def store():
                for i, r in enumerate(rows):
                    value, where = product[i * ROWS:(i + 1) * ROWS], (j, pl.ds(r, ROWS))
                    if r in fused:
                        value = value + other[where].astype(F32)
                    if r in alone or r in fused:
                        part[where] = value.astype(BF16)
                    else:
                        acc[where] = value

            return store

        def run(role, begin, end):
            loads, sends, held = {}, [], []
            for number, (kind, *args) in enumerate(programs[role][:end]):
                if kind == "load":
                    loads[args[0]] = load(role, *args)
                    if number >= begin:
                        for copy in loads[args[0]]:
                            copy.start()
                    if args[1] == "w1" and args[3] == [0]:
                        loads[args[0]].append(opening)
                elif kind == "loaded":
                    for copy in loads[args[0]]:
                        copy.wait()
                elif kind == "barrier":
                    pl.semaphore_wait(barrier, 2)
                elif kind == "cast":
                    r, k = args
                    x[k, pl.ds(r, ROWS)] = x_f32[pl.ds(r, ROWS), pl.ds(k * LANES, LANES)].astype(BF16)
                elif kind in ("hidden", "partial"):
                    held.append((hidden if kind == "hidden" else partial)(*args[1:]))
                    if not args[0]:
                        held.pop()()
                elif kind == "store":
                    while held:
                        held.pop(0)()
                elif kind == "add":
                    where = args[1], pl.ds(args[0], ROWS)
                    part[where] = (acc[where] + other[where].astype(F32)).astype(BF16)
                elif kind == "total":
                    r, j = args
                    value = part[j, pl.ds(r, ROWS)].astype(F32) + rest[j, pl.ds(r, ROWS)].astype(F32)
                    out[pl.ds(global_row(role, r), ROWS), pl.ds(j * LANES, LANES)] = value.astype(BF16)
                elif kind == "send":
                    slot, to, src, dst, r, n, j = args
                    row = global_row(role, r)
                    sends.append(pltpu.make_async_remote_copy(
                        tile(src, row if src == "out" else r, n, j),
                        tile(dst, r ^ HALF if to == 3 and dst != "out" else row, n, j),
                        send_sems.at[len(sends)],
                        recv_sems.at[slot + mirrored if role == SIDE else slot],
                        device_id=(to,), device_id_type=mesh))
                    sends[-1].start()
                elif kind == "recv":
                    slot, dst, r, n, j = args
                    landing = tile(dst, global_row(role, r) if dst == "out" else r, n, j)
                    pltpu.make_async_remote_copy(
                        landing, landing, send_sems.at[0], recv_sems.at[slot],
                        device_id=(me,), device_id_type=mesh).wait_recv()
                else:
                    while len(sends) > args[0]:
                        sends.pop(0).wait_send()

        roles = {SIDE: (me & 1) == 1, LAST: me == 2, FIRST: me == 0}
        head = {role: [step[0] in ("load", "store") for step in programs[role]].index(False)
                for role in roles}
        for role, mine in roles.items():
            pl.when(mine)(lambda role=role: run(role, 0, head[role]))
        for role, mine in roles.items():
            pl.when(mine)(lambda role=role: run(role, head[role], None))

    hbm = pl.BlockSpec(memory_space=pltpu.HBM)
    tiles = lambda blocks, dtype: pltpu.VMEM((blocks, 2 * HALF, LANES), dtype)
    return pl.pallas_call(
        body,
        out_shape=jax.ShapeDtypeStruct((512, 512), BF16),
        in_specs=[hbm, hbm, hbm],
        out_specs=pl.BlockSpec(memory_space=pltpu.VMEM),
        scratch_shapes=[
            pltpu.VMEM((512, 512 + LANES), F32),
            pltpu.VMEM((512, HIDDEN + LANES), F32),
            pltpu.VMEM((4, HIDDEN // 64, 64, LANES), F32),
            tiles(4, BF16),
            pltpu.VMEM((512, HIDDEN + LANES), F32),
            tiles(HIDDEN // LANES, BF16),
            tiles(4, F32),
            tiles(4, BF16),
            tiles(4, BF16),
            tiles(4, BF16),
            pltpu.SemaphoreType.DMA((count("load") + 1,)),
            pltpu.SemaphoreType.DMA((count("send"),)),
            pltpu.SemaphoreType.DMA((count("recv"),)),
        ],
        compiler_params=pltpu.CompilerParams(
            collective_id=0,
            vmem_limit_bytes=32 << 20,
            disable_bounds_checks=True,
            disable_semaphore_checks=True,
        ),
    )


def pallas_dist_mlp2_tp_i_m512_h1024_out512_kernel(x: jax.Array, W1: jax.Array, W2: jax.Array):
    return _build(_schedule(PLANS, VIA_FIRST))(x, W1, W2.reshape(HIDDEN // 64, 64, 512))
```
